```python
import numpy as np

kernel_name = "dist_layernorm_xy_m6144_n2048"

def setup_inputs():
    x = np.random.randn(12288, 4096).astype(np.float32)
    gamma = np.random.randn(4096).astype(np.float32)
    beta = np.random.randn(4096).astype(np.float32)
    return {"x": x, "gamma": gamma, "beta": beta}

def reference(x: np.ndarray, gamma: np.ndarray, beta: np.ndarray) -> np.ndarray:
    eps = 1e-5
    mean = np.mean(x, axis=1, keepdims=True)
    var = np.var(x, axis=1, keepdims=True)
    return gamma * (x - mean) / np.sqrt(var + eps) + beta
```

```python
import jax
import jax.numpy as jnp
from jax import lax
from jax.experimental import pallas as pl
from jax.experimental.pallas import tpu as pltpu

EPS = 1e-5

R1 = 256
R2 = 64
NC2 = 4
PREFETCH = 3
LAG1 = 1
LAG2 = 3


def pallas_dist_layernorm_xy_m6144_n2048_kernel(
    x: jax.Array,
    gamma: jax.Array,
    beta: jax.Array,
):
    M, N = x.shape
    M2 = R2 * NC2
    M1 = M - M2
    assert M1 > 0 and M1 % R1 == 0 and R1 % 8 == 0 and R2 % 8 == 0
    NC1 = M1 // R1
    NC = NC1 + NC2
    P = PREFETCH
    assert 2 * (R1 // 8) <= 128 and 2 * (R2 // 8) <= 128
    assert 1 <= P <= min(NC1, NC2) and 1 <= LAG1 < NC1 and LAG1 <= LAG2 <= NC2
    inv_n = 1.0 / N
    half_n = N / 2.0
    inv_2n = 1.0 / (2 * N)

    def body(x_hbm, g_hbm, b_hbm, out_ref, g_vmem, b_vmem, send_buf, recv_buf,
             in_sems, gb_sems, send_sems, recv_sems):
        my_x = lax.axis_index("x")
        my_y = lax.axis_index("y")
        nbr = (my_x, 1 - my_y)

        def aligned(v, m):
            return v if isinstance(v, int) else pl.multiple_of(v, m)

        def rows_of(phase):
            return R1 if phase == 1 else R2

        def first_row(phase, k):
            if phase == 1:
                return aligned(k * R1, R1)
            return aligned(M1 + k * R2, R2)

        def chunk_id(phase, k):
            return k if phase == 1 else NC1 + k

        def stat_rows(phase, k):
            return pl.ds(aligned(chunk_id(phase, k) * 8, 8), 8)

        def in_copy(phase, k):
            rows = pl.ds(first_row(phase, k), rows_of(phase))
            return pltpu.make_async_copy(
                x_hbm.at[rows], out_ref.at[rows], in_sems.at[chunk_id(phase, k)])

        def exchange(phase, k):
            c = chunk_id(phase, k)
            return pltpu.make_async_remote_copy(
                src_ref=send_buf.at[stat_rows(phase, k)],
                dst_ref=recv_buf.at[stat_rows(phase, k)],
                send_sem=send_sems.at[c],
                recv_sem=recv_sems.at[c],
                device_id=nbr,
                device_id_type=pl.DeviceIdType.MESH,
            )

        for k in range(P):
            in_copy(1, k).start()
        g_copy = pltpu.make_async_copy(g_hbm, g_vmem, gb_sems.at[0])
        b_copy = pltpu.make_async_copy(b_hbm, b_vmem, gb_sems.at[1])
        g_copy.start()
        b_copy.start()

        barrier = pltpu.get_barrier_semaphore()
        pl.semaphore_signal(barrier, inc=1, device_id=nbr,
                            device_id_type=pl.DeviceIdType.MESH)
        pl.semaphore_wait(barrier, 1)

        lane = lax.broadcasted_iota(jnp.int32, (8, 128), 1)

        def local_stats(phase, k):
            base = first_row(phase, k)
            packed = jnp.zeros((8, 128), jnp.float32)
            for t in range(rows_of(phase) // 8):
                xt = out_ref[pl.ds(base + 8 * t, 8), :]
                mean = jnp.sum(xt, axis=1, keepdims=True) * inv_n
                d = xt - mean
                m2 = jnp.sum(d * d, axis=1, keepdims=True)
                packed = jnp.where(lane == 2 * t, mean, packed)
                packed = jnp.where(lane == 2 * t + 1, m2, packed)
            send_buf[stat_rows(phase, k), :] = packed
            exchange(phase, k).start()

        def normalize(phase, k):
            base = first_row(phase, k)
            exchange(phase, k).wait_recv()
            loc = send_buf[stat_rows(phase, k), :]
            rem = recv_buf[stat_rows(phase, k), :]
            tot = loc + rem
            dlt = rem - loc
            corr = pltpu.roll(dlt * dlt * half_n, 1, axis=1)
            rstd = lax.rsqrt((tot + corr) * inv_2n + EPS)
            mean = tot * 0.5
            g = g_vmem[...]
            b = b_vmem[...]
            for t in range(rows_of(phase) // 8):
                rows = pl.ds(base + 8 * t, 8)
                xt = out_ref[rows, :]
                out_ref[rows, :] = (
                    (xt - mean[:, 2 * t:2 * t + 1]) * rstd[:, 2 * t + 1:2 * t + 2]
                ) * g + b

        def step1(i, carry):
            @pl.when(i + P < NC1)
            def _():
                in_copy(1, i + P).start()

            for q in range(P):
                @pl.when(i + P == NC1 + q)
                def _():
                    in_copy(2, q).start()

            in_copy(1, i).wait()
            local_stats(1, i)

            @pl.when(i == LAG1)
            def _():
                g_copy.wait()
                b_copy.wait()

            @pl.when(i >= LAG1)
            def _():
                normalize(1, i - LAG1)

            return carry

        lax.fori_loop(0, NC1, step1, 0)

        for q in range(LAG1):
            if q + P < NC2:
                in_copy(2, q + P).start()
            in_copy(2, q).wait()
            local_stats(2, q)
            normalize(1, NC1 - LAG1 + q)

        def step2(q, carry):
            @pl.when(q + P < NC2)
            def _():
                in_copy(2, q + P).start()

            in_copy(2, q).wait()
            local_stats(2, q)

            @pl.when(q >= LAG2)
            def _():
                normalize(2, q - LAG2)

            return carry

        lax.fori_loop(LAG1, NC2, step2, 0)
        for q in range(NC2 - LAG2, NC2):
            normalize(2, q)

        def drain1(i, carry):
            exchange(1, i).wait_send()
            return carry

        lax.fori_loop(0, NC1, drain1, 0)
        for q in range(NC2):
            exchange(2, q).wait_send()

    return pl.pallas_call(
        body,
        out_shape=pltpu.VMEM((M, N), jnp.float32),
        in_specs=[pl.BlockSpec(memory_space=pl.ANY)] * 3,
        out_specs=pl.BlockSpec(memory_space=pltpu.VMEM),
        scratch_shapes=[
            pltpu.VMEM((1, N), jnp.float32),
            pltpu.VMEM((1, N), jnp.float32),
            pltpu.VMEM((NC * 8, 128), jnp.float32),
            pltpu.VMEM((NC * 8, 128), jnp.float32),
            pltpu.SemaphoreType.DMA((NC,)),
            pltpu.SemaphoreType.DMA((2,)),
            pltpu.SemaphoreType.DMA((NC,)),
            pltpu.SemaphoreType.DMA((NC,)),
        ],
        compiler_params=pltpu.CompilerParams(
            collective_id=0,
            disable_semaphore_checks=True,
        ),
    )(x, gamma.reshape(1, N), beta.reshape(1, N))
```
